```python
import numpy as np

kernel_name = "dist_sum_ax0_xy_m2048_n1024"

def setup_inputs():
    return {"x": np.random.randn(4096, 2048).astype(np.float32)}

def reference(x: np.ndarray) -> np.ndarray:
    return np.sum(x, axis=0, keepdims=True)
```

```python
import jax
import jax.numpy as jnp
from jax import lax
from jax.experimental import pallas as pl
from jax.experimental.pallas import tpu as pltpu

_N_CHUNKS = 8


def pallas_dist_sum_ax0_xy_m2048_n1024_kernel(
    x: jax.Array,
):
    m, n = x.shape
    rows = m // _N_CHUNKS

    def kernel_body(x_ref, out_ref, buf, part, recv, load_sems, send_sem, recv_sem):
        my_x = lax.axis_index("x")
        my_y = lax.axis_index("y")
        peer = (1 - my_x, my_y)

        loads = [
            pltpu.make_async_copy(
                x_ref.at[pl.ds(i * rows, rows)],
                buf.at[pl.ds(i * rows, rows)],
                load_sems.at[i],
            )
            for i in range(_N_CHUNKS)
        ]
        for load in loads:
            load.start()

        barrier = pltpu.get_barrier_semaphore()
        pl.semaphore_signal(
            barrier, inc=1, device_id=peer, device_id_type=pl.DeviceIdType.MESH
        )

        acc = jnp.zeros((8, n), jnp.float32)
        for i in range(_N_CHUNKS):
            loads[i].wait()
            acc = acc + jnp.sum(
                buf[pl.ds(i * rows, rows), :].reshape(rows // 8, 8, n), axis=0
            )
        total = jnp.sum(acc, axis=0, keepdims=True)
        part[...] = total

        pl.semaphore_wait(barrier, 1)
        rdma = pltpu.make_async_remote_copy(
            src_ref=part,
            dst_ref=recv,
            send_sem=send_sem,
            recv_sem=recv_sem,
            device_id=peer,
            device_id_type=pl.DeviceIdType.MESH,
        )
        rdma.start()
        rdma.wait_recv()
        out_ref[...] = total + recv[...]
        rdma.wait_send()

    return pl.pallas_call(
        kernel_body,
        out_shape=jax.ShapeDtypeStruct((1, n), jnp.float32),
        in_specs=[pl.BlockSpec(memory_space=pltpu.HBM)],
        out_specs=pl.BlockSpec(memory_space=pltpu.VMEM),
        scratch_shapes=[
            pltpu.VMEM((m, n), jnp.float32),
            pltpu.VMEM((1, n), jnp.float32),
            pltpu.VMEM((1, n), jnp.float32),
            pltpu.SemaphoreType.DMA((_N_CHUNKS,)),
            pltpu.SemaphoreType.DMA,
            pltpu.SemaphoreType.DMA,
        ],
        compiler_params=pltpu.CompilerParams(
            collective_id=0, vmem_limit_bytes=32 * 1024 * 1024
        ),
    )(x)
```

```python
import jax
import jax.numpy as jnp
from jax import lax
from jax.experimental import pallas as pl
from jax.experimental.pallas import tpu as pltpu

_SUBLANES = 8
_LANES = 128

_DETOUR_ROWS = 56
_PUSHED_PIECES = (112, 8)
_N_LARGE_PIECES = 4
_SMALL_PIECES = (96, 24, 8)
_COLUMN_GROUPS = ((6, (72, 24)), (1, (72, 24)), (1, (64, 16, 16)))


def _spans(sizes):
    spans, start = [], 0
    for size in sizes:
        spans.append((start, size))
        start += size
    return spans


def _tree_sum(terms):
    while len(terms) > 1:
        pairs = [terms[i] + terms[i + 1] for i in range(0, len(terms) - 1, 2)]
        terms = pairs + terms[2 * len(pairs) :]
    return terms[0]


def _add_rows(acc, ref, start, rows, block):
    cols = pl.ds(block * _LANES, _LANES)
    terms = [] if acc is None else [acc]
    if rows <= 128:
        terms += [
            ref[pl.ds(r, _SUBLANES), cols]
            for r in range(start, start + rows, _SUBLANES)
        ]
    else:
        tiles = ref[pl.ds(start, rows), cols].reshape(-1, _SUBLANES, _LANES)
        terms.append(jnp.sum(tiles, axis=0))
    return _tree_sum(terms)


def _sum_sublanes(accs):
    count = len(accs)
    if count == 1:
        return jnp.sum(accs[0], axis=0, keepdims=True)
    row = lax.broadcasted_iota(jnp.int32, (_SUBLANES, _LANES), 0)
    step = 1
    while step < _SUBLANES:
        first = (row & step) == 0
        merged = []
        for i in range(0, len(accs), 2):
            if i + 1 < len(accs):
                kept = jnp.where(first, accs[i], accs[i + 1])
                moved = jnp.where(first, accs[i + 1], accs[i])
            else:
                kept = moved = accs[i]
            merged.append(kept + pltpu.roll(moved, _SUBLANES - step, 0))
        accs = merged
        step *= 2
    return accs[0][:count]


def pallas_dist_sum_ax0_xy_m2048_n1024_kernel(
    x: jax.Array,
):
    m, n = x.shape
    n_blocks = n // _LANES
    assert n_blocks == _SUBLANES == sum(width for width, _ in _COLUMN_GROUPS)

    pushed_rows = sum(_PUSHED_PIECES)
    last_rows = sum(_COLUMN_GROUPS[0][1])
    main_rows = m - _DETOUR_ROWS - pushed_rows - last_rows
    main_start = _DETOUR_ROWS
    pushed_start = main_start + main_rows
    last_start = pushed_start + pushed_rows

    large_rows = main_rows - sum(_SMALL_PIECES)
    large = large_rows // _N_LARGE_PIECES // _SUBLANES * _SUBLANES
    main_spans = _spans(
        [large_rows - (_N_LARGE_PIECES - 1) * large]
        + [large] * (_N_LARGE_PIECES - 1)
        + list(_SMALL_PIECES)
    )
    pushed_spans = _spans(_PUSHED_PIECES)
    n_groups = len(_COLUMN_GROUPS)
    max_group_pieces = max(len(pieces) for _, pieces in _COLUMN_GROUPS)

    def kernel_body(
        x_ref,
        out_ref,
        main_buf,
        detour_smem,
        detour_buf,
        own_pushed_buf,
        peer_pushed_buf,
        group_bufs,
        send_bufs,
        recv_bufs,
        main_sems,
        group_sems,
        local_sems,
        push_send_sems,
        push_recv_sems,
        sum_send_sems,
        sum_recv_sems,
    ):
        main_copies = [
            pltpu.make_async_copy(
                x_ref.at[pl.ds(main_start + start, rows)],
                main_buf.at[pl.ds(start, rows)],
                main_sems.at[i],
            )
            for i, (start, rows) in enumerate(main_spans)
        ]
        detour_in = pltpu.make_async_copy(
            x_ref.at[pl.ds(0, _DETOUR_ROWS)], detour_smem, local_sems.at[0]
        )
        detour_out = pltpu.make_async_copy(detour_smem, detour_buf, local_sems.at[1])
        own_pushed = pltpu.make_async_copy(
            x_ref.at[pl.ds(pushed_start, pushed_rows)],
            own_pushed_buf,
            local_sems.at[2],
        )
        group_copies = []
        block = 0
        for g, (width, pieces) in enumerate(_COLUMN_GROUPS):
            group_copies.append(
                [
                    pltpu.make_async_copy(
                        x_ref.at[
                            pl.ds(last_start + start, rows),
                            pl.ds(block * _LANES, width * _LANES),
                        ],
                        group_bufs[g].at[pl.ds(start, rows)],
                        group_sems.at[g * max_group_pieces + i],
                    )
                    for i, (start, rows) in enumerate(_spans(pieces))
                ]
            )
            block += width

        main_copies[0].start()
        detour_in.start()
        for copy in main_copies[1:]:
            copy.start()
        for copies in group_copies:
            for copy in copies:
                copy.start()

        peer = (1 - lax.axis_index("x"), lax.axis_index("y"))

        def to_peer(src, dst, send_sem, recv_sem):
            return pltpu.make_async_remote_copy(
                src_ref=src,
                dst_ref=dst,
                send_sem=send_sem,
                recv_sem=recv_sem,
                device_id=peer,
                device_id_type=pl.DeviceIdType.MESH,
            )

        barrier = pltpu.get_barrier_semaphore()
        pl.semaphore_signal(
            barrier, inc=1, device_id=peer, device_id_type=pl.DeviceIdType.MESH
        )
        pl.semaphore_wait(barrier, 1)

        pushes = [
            to_peer(
                x_ref.at[pl.ds(pushed_start + start, rows)],
                peer_pushed_buf.at[pl.ds(start, rows)],
                push_send_sems.at[i],
                push_recv_sems.at[i],
            )
            for i, (start, rows) in enumerate(pushed_spans)
        ]
        for push in pushes:
            push.start()

        def add_all_blocks(accs, ref, start, rows):
            return [
                _add_rows(acc, ref, start, rows, j) for j, acc in enumerate(accs)
            ]

        accs = [None] * n_blocks
        for i, ((start, rows), copy) in enumerate(zip(main_spans, main_copies)):
            if i == 1:
                detour_in.wait()
                detour_out.start()
            if i == _N_LARGE_PIECES:
                detour_out.wait()
                accs = add_all_blocks(accs, detour_buf, 0, _DETOUR_ROWS)
            copy.wait()
            accs = add_all_blocks(accs, main_buf, start, rows)

        sums, sends = [], []
        block = 0
        for g, (width, pieces) in enumerate(_COLUMN_GROUPS):
            group = accs[block : block + width]
            for (start, rows), copy in zip(_spans(pieces), group_copies[g]):
                copy.wait()
                group = add_all_blocks(group, group_bufs[g], start, rows)
            sums.append(_sum_sublanes(group))
            send_bufs[g][...] = sums[g]
            send = to_peer(
                send_bufs[g], recv_bufs[g], sum_send_sems.at[g], sum_recv_sems.at[g]
            )
            send.start()
            sends.append(send)
            block += width

        own_pushed.start()
        own_pushed.wait()
        late = add_all_blocks([None] * n_blocks, own_pushed_buf, 0, pushed_rows)
        for (start, rows), push in zip(pushed_spans, pushes):
            push.wait_recv()
            late = add_all_blocks(late, peer_pushed_buf, start, rows)
        block = 0
        for g, (width, _) in enumerate(_COLUMN_GROUPS):
            sums[g] = sums[g] + _sum_sublanes(late[block : block + width])
            block += width

        for copy in pushes + sends:
            copy.wait_send()
        block = 0
        for g, (width, _) in enumerate(_COLUMN_GROUPS):
            sends[g].wait_recv()
            out_ref[pl.ds(block, width), :] = sums[g] + recv_bufs[g][...]
            block += width

    def vmem(*shape):
        return pltpu.VMEM(shape, jnp.float32)

    out = pl.pallas_call(
        kernel_body,
        out_shape=jax.ShapeDtypeStruct((n_blocks, _LANES), jnp.float32),
        in_specs=[pl.BlockSpec(memory_space=pltpu.HBM)],
        out_specs=pl.BlockSpec(memory_space=pltpu.VMEM),
        scratch_shapes=[
            vmem(main_rows, n),
            pltpu.SMEM((_DETOUR_ROWS, n), jnp.float32),
            vmem(_DETOUR_ROWS, n),
            vmem(pushed_rows, n),
            vmem(pushed_rows, n),
            [vmem(last_rows, width * _LANES) for width, _ in _COLUMN_GROUPS],
            [vmem(width, _LANES) for width, _ in _COLUMN_GROUPS],
            [vmem(width, _LANES) for width, _ in _COLUMN_GROUPS],
            pltpu.SemaphoreType.DMA((len(main_spans),)),
            pltpu.SemaphoreType.DMA((n_groups * max_group_pieces,)),
            pltpu.SemaphoreType.DMA((3,)),
            pltpu.SemaphoreType.DMA((len(pushed_spans),)),
            pltpu.SemaphoreType.DMA((len(pushed_spans),)),
            pltpu.SemaphoreType.DMA((n_groups,)),
            pltpu.SemaphoreType.DMA((n_groups,)),
        ],
        compiler_params=pltpu.CompilerParams(
            collective_id=0,
            vmem_limit_bytes=32 * 1024 * 1024,
            disable_semaphore_checks=True,
        ),
    )(x)
    return out.reshape(1, n)
```

```python
import jax
import jax.numpy as jnp
from jax import lax
from jax.experimental import pallas as pl
from jax.experimental.pallas import tpu as pltpu

_SUBLANES = 8
_LANES = 128

_SEGMENTS = 16
_DETOUR_ROWS = 56
_PUSHED_ROWS = 120
_COLUMN_GROUPS = ((6, (13, 3)), (1, (13, 3)), (1, (12, 2, 2)))


def _spans(sizes):
    spans, start = [], 0
    for size in sizes:
        spans.append((start, size))
        start += size
    return spans


def _tree_sum(terms):
    while len(terms) > 1:
        pairs = [terms[i] + terms[i + 1] for i in range(0, len(terms) - 1, 2)]
        terms = pairs + terms[2 * len(pairs) :]
    return terms[0]


def _add_tiles(accs, ref, start, count):
    return [
        _tree_sum(
            ([] if acc is None else [acc])
            + [
                ref[k, :, pl.ds(j * _LANES, _LANES)]
                for k in range(start, start + count)
            ]
        )
        for j, acc in enumerate(accs)
    ]


def _sum_sublanes(accs):
    count = len(accs)
    if count == 1:
        return jnp.sum(accs[0], axis=0, keepdims=True)
    row = lax.broadcasted_iota(jnp.int32, (_SUBLANES, _LANES), 0)
    step = 1
    while step < _SUBLANES:
        first = (row & step) == 0
        merged = []
        for i in range(0, len(accs), 2):
            if i + 1 < len(accs):
                kept = jnp.where(first, accs[i], accs[i + 1])
                moved = jnp.where(first, accs[i + 1], accs[i])
            else:
                kept = moved = accs[i]
            merged.append(kept + pltpu.roll(moved, _SUBLANES - step, 0))
        accs = merged
        step *= 2
    return accs[0][:count]


def pallas_dist_sum_ax0_xy_m2048_n1024_kernel(
    x: jax.Array,
):
    m, n = x.shape
    n_blocks = n // _LANES
    assert n_blocks == _SUBLANES == sum(width for width, _ in _COLUMN_GROUPS)

    n_steps = m // (_SEGMENTS * _SUBLANES)
    detour_strips = _DETOUR_ROWS // _SUBLANES
    pushed_strips = _PUSHED_ROWS // _SUBLANES
    assert max(detour_strips, pushed_strips) < n_steps
    step_spans = []
    for step in range(n_steps - 1):
        first = 1 if step < detour_strips else 0
        end = _SEGMENTS - 1 if step < pushed_strips else _SEGMENTS
        step_spans.append((first, end - first))
    n_groups = len(_COLUMN_GROUPS)
    n_loads = len(step_spans) + sum(len(pieces) for _, pieces in _COLUMN_GROUPS)

    def kernel_body(
        x_ref,
        out_ref,
        main_buf,
        detour_smem,
        detour_buf,
        own_pushed_buf,
        peer_pushed_buf,
        group_bufs,
        send_bufs,
        recv_bufs,
        load_sems,
        late_sems,
        push_sems,
        sum_send_sems,
        sum_recv_sems,
    ):
        next_sem = iter(range(n_loads + 1))
        step_copies = [
            pltpu.make_async_copy(
                x_ref.at[pl.ds(first, count), step],
                main_buf.at[step, pl.ds(first, count)],
                load_sems.at[next(next_sem)],
            )
            for step, (first, count) in enumerate(step_spans)
        ]
        detour_in = pltpu.make_async_copy(
            x_ref.at[0, pl.ds(0, detour_strips)],
            detour_smem,
            load_sems.at[next(next_sem)],
        )
        group_copies = []
        block = 0
        for g, (width, pieces) in enumerate(_COLUMN_GROUPS):
            group_copies.append(
                [
                    pltpu.make_async_copy(
                        x_ref.at[
                            pl.ds(first, count),
                            n_steps - 1,
                            :,
                            pl.ds(block * _LANES, width * _LANES),
                        ],
                        group_bufs[g].at[pl.ds(first, count)],
                        load_sems.at[next(next_sem)],
                    )
                    for first, count in _spans(pieces)
                ]
            )
            block += width
        detour_out = pltpu.make_async_copy(detour_smem, detour_buf, late_sems.at[0])
        pushed = x_ref.at[_SEGMENTS - 1, pl.ds(0, pushed_strips)]
        own_pushed = pltpu.make_async_copy(pushed, own_pushed_buf, late_sems.at[1])

        step_copies[0].start()
        detour_in.start()
        for copy in step_copies[1:]:
            copy.start()
        for copies in group_copies:
            for copy in copies:
                copy.start()

        peer = (1 - lax.axis_index("x"), lax.axis_index("y"))

        def to_peer(src, dst, send_sem, recv_sem):
            return pltpu.make_async_remote_copy(
                src_ref=src,
                dst_ref=dst,
                send_sem=send_sem,
                recv_sem=recv_sem,
                device_id=peer,
                device_id_type=pl.DeviceIdType.MESH,
            )

        barrier = pltpu.get_barrier_semaphore()
        pl.semaphore_signal(
            barrier, inc=1, device_id=peer, device_id_type=pl.DeviceIdType.MESH
        )
        pl.semaphore_wait(barrier, 1)
        push = to_peer(pushed, peer_pushed_buf, push_sems.at[0], push_sems.at[1])
        push.start()

        accs = [None] * n_blocks
        for step, ((first, count), copy) in enumerate(zip(step_spans, step_copies)):
            if step == n_steps // 2 - 1:
                detour_in.wait()
                detour_out.start()
            if step == n_steps - 2:
                detour_out.wait()
                accs = _add_tiles(accs, detour_buf, 0, detour_strips)
            copy.wait()
            accs = _add_tiles(accs, main_buf.at[step], first, count)

        sums, sends = [], []
        block = 0
        for g, (width, pieces) in enumerate(_COLUMN_GROUPS):
            group = accs[block : block + width]
            for (first, count), copy in zip(_spans(pieces), group_copies[g]):
                copy.wait()
                group = _add_tiles(group, group_bufs[g], first, count)
            sums.append(_sum_sublanes(group))
            send_bufs[g][...] = sums[g]
            send = to_peer(
                send_bufs[g], recv_bufs[g], sum_send_sems.at[g], sum_recv_sems.at[g]
            )
            send.start()
            sends.append(send)
            block += width

        own_pushed.start()
        own_pushed.wait()
        late = _add_tiles([None] * n_blocks, own_pushed_buf, 0, pushed_strips)
        push.wait_recv()
        late = _add_tiles(late, peer_pushed_buf, 0, pushed_strips)
        block = 0
        for g, (width, _) in enumerate(_COLUMN_GROUPS):
            sums[g] = sums[g] + _sum_sublanes(late[block : block + width])
            block += width

        for copy in [push] + sends:
            copy.wait_send()
        block = 0
        for g, (width, _) in enumerate(_COLUMN_GROUPS):
            sends[g].wait_recv()
            out_ref[pl.ds(block, width), :] = sums[g] + recv_bufs[g][...]
            block += width

    def strips(count, width=n):
        return pltpu.VMEM((count, _SUBLANES, width), jnp.float32)

    sum_bufs = [
        pltpu.VMEM((width, _LANES), jnp.float32) for width, _ in _COLUMN_GROUPS
    ]
    out = pl.pallas_call(
        kernel_body,
        out_shape=jax.ShapeDtypeStruct((n_blocks, _LANES), jnp.float32),
        in_specs=[pl.BlockSpec(memory_space=pltpu.HBM)],
        out_specs=pl.BlockSpec(memory_space=pltpu.VMEM),
        scratch_shapes=[
            pltpu.VMEM((n_steps - 1, _SEGMENTS, _SUBLANES, n), jnp.float32),
            pltpu.SMEM((detour_strips, _SUBLANES, n), jnp.float32),
            strips(detour_strips),
            strips(pushed_strips),
            strips(pushed_strips),
            [strips(_SEGMENTS, width * _LANES) for width, _ in _COLUMN_GROUPS],
            sum_bufs,
            sum_bufs,
            pltpu.SemaphoreType.DMA((n_loads + 1,)),
            pltpu.SemaphoreType.DMA((2,)),
            pltpu.SemaphoreType.DMA((2,)),
            pltpu.SemaphoreType.DMA((n_groups,)),
            pltpu.SemaphoreType.DMA((n_groups,)),
        ],
        compiler_params=pltpu.CompilerParams(
            collective_id=0, disable_semaphore_checks=True
        ),
    )(x.reshape(_SEGMENTS, n_steps, _SUBLANES, n))
    return out.reshape(1, n)
```

```python
import jax
import jax.numpy as jnp
from jax import lax
from jax.experimental import pallas as pl
from jax.experimental.pallas import tpu as pltpu

_SUBLANES = 8
_LANES = 128

_SEGMENTS = 16
_DETOUR_STRIPS = 3
_DETOUR_STEP = 10
_PUSHED_STRIPS = 15
_GROUP_WIDTHS = (6, 1, 1)
_GROUP_PIECES = (9, 3)


def _tree_sum(terms):
    while len(terms) > 1:
        pairs = [terms[i] + terms[i + 1] for i in range(0, len(terms) - 1, 2)]
        terms = pairs + terms[2 * len(pairs) :]
    return terms[0]


def _add_strips(accs, ref, first, count):
    return [
        _tree_sum(
            ([] if acc is None else [acc])
            + [
                ref[k, :, pl.ds(j * _LANES, _LANES)]
                for k in range(first, first + count)
            ]
        )
        for j, acc in enumerate(accs)
    ]


def _sum_sublanes(accs):
    count = len(accs)
    if count == 1:
        return jnp.sum(accs[0], axis=0, keepdims=True)
    row = lax.broadcasted_iota(jnp.int32, (_SUBLANES, _LANES), 0)
    step = 1
    while step < _SUBLANES:
        first = (row & step) == 0
        merged = []
        for i in range(0, len(accs), 2):
            if i + 1 < len(accs):
                kept = jnp.where(first, accs[i], accs[i + 1])
                moved = jnp.where(first, accs[i + 1], accs[i])
            else:
                kept = moved = accs[i]
            merged.append(kept + pltpu.roll(moved, _SUBLANES - step, 0))
        accs = merged
        step *= 2
    return accs[0][:count]


def pallas_dist_sum_ax0_xy_m2048_n1024_kernel(
    x: jax.Array,
):
    m, n = x.shape
    n_blocks = n // _LANES
    n_steps = m // (_SEGMENTS * _SUBLANES)
    group_segments = sum(_GROUP_PIECES)
    assert n_blocks == _SUBLANES == sum(_GROUP_WIDTHS)
    assert max(_DETOUR_STRIPS, _DETOUR_STEP, _PUSHED_STRIPS) < n_steps
    assert group_segments < _SEGMENTS

    step_spans = []
    for step in range(n_steps - 1):
        first = 1 if step < _DETOUR_STRIPS else 0
        end = _SEGMENTS - 1 if step < _PUSHED_STRIPS else _SEGMENTS
        step_spans.append((first, end - first))
    step_spans.append((0, _SEGMENTS - group_segments))
    groups = [
        (sum(_GROUP_WIDTHS[:g]), width) for g, width in enumerate(_GROUP_WIDTHS)
    ]
    pieces = [
        (sum(_GROUP_PIECES[:i]), count) for i, count in enumerate(_GROUP_PIECES)
    ]
    n_loads = n_steps + 1 + len(groups) * len(pieces)

    def kernel_body(
        x_ref,
        out_ref,
        main_buf,
        detour_smem,
        detour_buf,
        own_pushed_buf,
        peer_pushed_buf,
        group_bufs,
        send_bufs,
        recv_bufs,
        load_sems,
        late_sems,
        push_sems,
        sum_send_sems,
        sum_recv_sems,
    ):
        next_sem = iter(range(n_loads))
        step_copies = [
            pltpu.make_async_copy(
                x_ref.at[pl.ds(first, count), step],
                main_buf.at[step, pl.ds(first, count)],
                load_sems.at[next(next_sem)],
            )
            for step, (first, count) in enumerate(step_spans)
        ]
        detour_in = pltpu.make_async_copy(
            x_ref.at[0, pl.ds(0, _DETOUR_STRIPS)],
            detour_smem,
            load_sems.at[next(next_sem)],
        )
        group_copies = [
            [
                pltpu.make_async_copy(
                    x_ref.at[
                        pl.ds(_SEGMENTS - group_segments + first, count),
                        n_steps - 1,
                        :,
                        pl.ds(block * _LANES, width * _LANES),
                    ],
                    group_bufs[g].at[pl.ds(first, count)],
                    load_sems.at[next(next_sem)],
                )
                for first, count in pieces
            ]
            for g, (block, width) in enumerate(groups)
        ]
        detour_out = pltpu.make_async_copy(detour_smem, detour_buf, late_sems.at[0])
        pushed = x_ref.at[_SEGMENTS - 1, pl.ds(0, _PUSHED_STRIPS)]
        own_pushed = pltpu.make_async_copy(pushed, own_pushed_buf, late_sems.at[1])

        step_copies[0].start()
        detour_in.start()
        for copy in step_copies[1:]:
            copy.start()
        for copies in group_copies:
            for copy in copies:
                copy.start()

        peer = (1 - lax.axis_index("x"), lax.axis_index("y"))

        def to_peer(src, dst, send_sem, recv_sem):
            return pltpu.make_async_remote_copy(
                src_ref=src,
                dst_ref=dst,
                send_sem=send_sem,
                recv_sem=recv_sem,
                device_id=peer,
                device_id_type=pl.DeviceIdType.MESH,
            )

        barrier = pltpu.get_barrier_semaphore()
        pl.semaphore_signal(
            barrier, inc=1, device_id=peer, device_id_type=pl.DeviceIdType.MESH
        )
        pl.semaphore_wait(barrier, 1)
        push = to_peer(pushed, peer_pushed_buf, push_sems.at[0], push_sems.at[1])
        push.start()

        accs = [None] * n_blocks
        for step, ((first, count), copy) in enumerate(zip(step_spans, step_copies)):
            if step == _DETOUR_STEP:
                detour_in.wait()
                detour_out.start()
            if step == n_steps - 1:
                detour_out.wait()
                accs = _add_strips(accs, detour_buf, 0, _DETOUR_STRIPS)
            copy.wait()
            accs = _add_strips(accs, main_buf.at[step], first, count)

        sums, sends = [], []
        for g, (block, width) in enumerate(groups):
            group = accs[block : block + width]
            for (first, count), copy in zip(pieces, group_copies[g]):
                copy.wait()
                group = _add_strips(group, group_bufs[g], first, count)
            sums.append(_sum_sublanes(group))
            send_bufs[g][...] = sums[g]
            send = to_peer(
                send_bufs[g], recv_bufs[g], sum_send_sems.at[g], sum_recv_sems.at[g]
            )
            send.start()
            sends.append(send)

        own_pushed.start()
        own_pushed.wait()
        late = _add_strips([None] * n_blocks, own_pushed_buf, 0, _PUSHED_STRIPS)
        push.wait_recv()
        late = _add_strips(late, peer_pushed_buf, 0, _PUSHED_STRIPS)
        for g, (block, width) in enumerate(groups):
            sums[g] = sums[g] + _sum_sublanes(late[block : block + width])

        for copy in [push] + sends:
            copy.wait_send()
        for g, (block, width) in enumerate(groups):
            sends[g].wait_recv()
            out_ref[pl.ds(block, width), :] = sums[g] + recv_bufs[g][...]

    def strips(count, width=n):
        return pltpu.VMEM((count, _SUBLANES, width), jnp.float32)

    sum_bufs = [pltpu.VMEM((width, _LANES), jnp.float32) for width in _GROUP_WIDTHS]
    out = pl.pallas_call(
        kernel_body,
        out_shape=jax.ShapeDtypeStruct((n_blocks, _LANES), jnp.float32),
        in_specs=[pl.BlockSpec(memory_space=pltpu.HBM)],
        out_specs=pl.BlockSpec(memory_space=pltpu.VMEM),
        scratch_shapes=[
            pltpu.VMEM((n_steps, _SEGMENTS, _SUBLANES, n), jnp.float32),
            pltpu.SMEM((_DETOUR_STRIPS, _SUBLANES, n), jnp.float32),
            strips(_DETOUR_STRIPS),
            strips(_PUSHED_STRIPS),
            strips(_PUSHED_STRIPS),
            [strips(group_segments, width * _LANES) for width in _GROUP_WIDTHS],
            sum_bufs,
            sum_bufs,
            pltpu.SemaphoreType.DMA((n_loads,)),
            pltpu.SemaphoreType.DMA((2,)),
            pltpu.SemaphoreType.DMA((2,)),
            pltpu.SemaphoreType.DMA((len(groups),)),
            pltpu.SemaphoreType.DMA((len(groups),)),
        ],
        compiler_params=pltpu.CompilerParams(
            collective_id=0, disable_semaphore_checks=True
        ),
    )(x.reshape(_SEGMENTS, n_steps, _SUBLANES, n))
    return out.reshape(1, n)
```

```python
import jax
import jax.numpy as jnp
from jax import lax
from jax.experimental import pallas as pl
from jax.experimental.pallas import tpu as pltpu

_SUBLANES = 8
_LANES = 128

_SEGMENTS = 16
_FIRST_STRIP = 7
_DETOUR_STRIPS = 3
_DETOUR_STEP = 10
_PUSHED_STRIPS = 15
_GROUP_WIDTHS = (6, 1, 1)
_GROUP_PIECES = (9, 3)


def _tree_sum(terms):
    while len(terms) > 1:
        pairs = [terms[i] + terms[i + 1] for i in range(0, len(terms) - 1, 2)]
        terms = pairs + terms[2 * len(pairs) :]
    return terms[0]


def _add_strips(accs, ref, first, count):
    return [
        _tree_sum(
            ([] if acc is None else [acc])
            + [
                ref[k, :, pl.ds(j * _LANES, _LANES)]
                for k in range(first, first + count)
            ]
        )
        for j, acc in enumerate(accs)
    ]


def _sum_sublanes(accs):
    count = len(accs)
    if count == 1:
        return jnp.sum(accs[0], axis=0, keepdims=True)
    row = lax.broadcasted_iota(jnp.int32, (_SUBLANES, _LANES), 0)
    step = 1
    while step < _SUBLANES:
        first = (row & step) == 0
        merged = []
        for i in range(0, len(accs), 2):
            if i + 1 < len(accs):
                kept = jnp.where(first, accs[i], accs[i + 1])
                moved = jnp.where(first, accs[i + 1], accs[i])
            else:
                kept = moved = accs[i]
            merged.append(kept + pltpu.roll(moved, _SUBLANES - step, 0))
        accs = merged
        step *= 2
    return accs[0][:count]


def pallas_dist_sum_ax0_xy_m2048_n1024_kernel(
    x: jax.Array,
):
    m, n = x.shape
    n_blocks = n // _LANES
    n_steps = m // (_SEGMENTS * _SUBLANES)
    group_segments = sum(_GROUP_PIECES)
    assert n_blocks == _SUBLANES == sum(_GROUP_WIDTHS)
    assert max(_DETOUR_STRIPS, _DETOUR_STEP, _PUSHED_STRIPS) < n_steps

    steps = []
    for step in range(n_steps):
        strip = (_FIRST_STRIP + step) % n_steps
        first = 1 if strip < _DETOUR_STRIPS else 0
        end = _SEGMENTS - 1 if strip < _PUSHED_STRIPS else _SEGMENTS
        if step == n_steps - 1:
            assert first == 0 and group_segments < end
            first = group_segments
        steps.append((strip, first, end - first))
    last_strip = steps[-1][0]
    groups = [
        (sum(_GROUP_WIDTHS[:g]), width) for g, width in enumerate(_GROUP_WIDTHS)
    ]
    pieces = [
        (sum(_GROUP_PIECES[:i]), count) for i, count in enumerate(_GROUP_PIECES)
    ]
    n_loads = n_steps + 1 + len(groups) * len(pieces)

    def kernel_body(
        x_ref,
        out_ref,
        main_buf,
        detour_smem,
        detour_buf,
        own_pushed_buf,
        peer_pushed_buf,
        group_bufs,
        send_bufs,
        recv_bufs,
        load_sems,
        late_sems,
        push_sems,
        sum_send_sems,
        sum_recv_sems,
    ):
        next_sem = iter(range(n_loads))
        step_copies = [
            pltpu.make_async_copy(
                x_ref.at[pl.ds(first, count), strip],
                main_buf.at[strip, pl.ds(first, count)],
                load_sems.at[next(next_sem)],
            )
            for strip, first, count in steps
        ]
        detour_in = pltpu.make_async_copy(
            x_ref.at[0, pl.ds(0, _DETOUR_STRIPS)],
            detour_smem,
            load_sems.at[next(next_sem)],
        )
        group_copies = [
            [
                pltpu.make_async_copy(
                    x_ref.at[
                        pl.ds(first, count),
                        last_strip,
                        :,
                        pl.ds(block * _LANES, width * _LANES),
                    ],
                    group_bufs[g].at[pl.ds(first, count)],
                    load_sems.at[next(next_sem)],
                )
                for first, count in pieces
            ]
            for g, (block, width) in enumerate(groups)
        ]
        detour_out = pltpu.make_async_copy(detour_smem, detour_buf, late_sems.at[0])
        pushed = x_ref.at[_SEGMENTS - 1, pl.ds(0, _PUSHED_STRIPS)]
        own_pushed = pltpu.make_async_copy(pushed, own_pushed_buf, late_sems.at[1])

        step_copies[0].start()
        detour_in.start()
        for copy in step_copies[1:]:
            copy.start()
        for copies in group_copies:
            for copy in copies:
                copy.start()

        peer = (1 - lax.axis_index("x"), lax.axis_index("y"))

        def to_peer(src, dst, send_sem, recv_sem):
            return pltpu.make_async_remote_copy(
                src_ref=src,
                dst_ref=dst,
                send_sem=send_sem,
                recv_sem=recv_sem,
                device_id=peer,
                device_id_type=pl.DeviceIdType.MESH,
            )

        barrier = pltpu.get_barrier_semaphore()
        pl.semaphore_signal(
            barrier, inc=1, device_id=peer, device_id_type=pl.DeviceIdType.MESH
        )
        pl.semaphore_wait(barrier, 1)
        push = to_peer(pushed, peer_pushed_buf, push_sems.at[0], push_sems.at[1])
        push.start()

        accs = [None] * n_blocks
        for step, (strip, first, count) in enumerate(steps):
            if step == _DETOUR_STEP:
                detour_in.wait()
                detour_out.start()
            if step == n_steps - 1:
                detour_out.wait()
                accs = _add_strips(accs, detour_buf, 0, _DETOUR_STRIPS)
            step_copies[step].wait()
            accs = _add_strips(accs, main_buf.at[strip], first, count)

        sums, sends = [], []
        for g, (block, width) in enumerate(groups):
            group = accs[block : block + width]
            for (first, count), copy in zip(pieces, group_copies[g]):
                copy.wait()
                group = _add_strips(group, group_bufs[g], first, count)
            sums.append(_sum_sublanes(group))
            send_bufs[g][...] = sums[g]
            send = to_peer(
                send_bufs[g], recv_bufs[g], sum_send_sems.at[g], sum_recv_sems.at[g]
            )
            send.start()
            sends.append(send)

        own_pushed.start()
        own_pushed.wait()
        late = _add_strips([None] * n_blocks, own_pushed_buf, 0, _PUSHED_STRIPS)
        push.wait_recv()
        late = _add_strips(late, peer_pushed_buf, 0, _PUSHED_STRIPS)
        for g, (block, width) in enumerate(groups):
            sums[g] = sums[g] + _sum_sublanes(late[block : block + width])

        for copy in [push] + sends:
            copy.wait_send()
        for g, (block, width) in enumerate(groups):
            sends[g].wait_recv()
            out_ref[pl.ds(block, width), :] = sums[g] + recv_bufs[g][...]

    def strips(count, width=n):
        return pltpu.VMEM((count, _SUBLANES, width), jnp.float32)

    sum_bufs = [pltpu.VMEM((width, _LANES), jnp.float32) for width in _GROUP_WIDTHS]
    out = pl.pallas_call(
        kernel_body,
        out_shape=jax.ShapeDtypeStruct((n_blocks, _LANES), jnp.float32),
        in_specs=[pl.BlockSpec(memory_space=pltpu.HBM)],
        out_specs=pl.BlockSpec(memory_space=pltpu.VMEM),
        scratch_shapes=[
            pltpu.VMEM((n_steps, _SEGMENTS, _SUBLANES, n), jnp.float32),
            pltpu.SMEM((_DETOUR_STRIPS, _SUBLANES, n), jnp.float32),
            strips(_DETOUR_STRIPS),
            strips(_PUSHED_STRIPS),
            strips(_PUSHED_STRIPS),
            [strips(group_segments, width * _LANES) for width in _GROUP_WIDTHS],
            sum_bufs,
            sum_bufs,
            pltpu.SemaphoreType.DMA((n_loads,)),
            pltpu.SemaphoreType.DMA((2,)),
            pltpu.SemaphoreType.DMA((2,)),
            pltpu.SemaphoreType.DMA((len(groups),)),
            pltpu.SemaphoreType.DMA((len(groups),)),
        ],
        compiler_params=pltpu.CompilerParams(
            collective_id=0, disable_semaphore_checks=True
        ),
    )(x.reshape(_SEGMENTS, n_steps, _SUBLANES, n))
    return out.reshape(1, n)
```
